```python
import numpy as np

kernel_name = "dist_f_of_ar_i_m4096_n1024"

def setup_inputs():
    t = np.random.randn(16384, 1024).astype(np.float32)
    return {"t": t}

def reference(t: np.ndarray) -> np.ndarray:
    s = t.reshape(4, 4096, 1024).sum(axis=0)
    r = np.maximum(s, 0.0)
    return np.tanh(s) * s * s + r * r * r
```

```python
import itertools

import jax
import jax.numpy as jnp
from jax import lax
from jax.experimental import pallas as pl
from jax.experimental.pallas import tpu as pltpu

_TILE = 16

_RS1_FIRST = (16, 32, 80, 128, 256)
_RS1_SECOND = (512,)
_RS2 = (128, 128, 128, 128)
_AG2_LAST = (256, 128, 64, 48, 16)


def _spans(sizes):
    ends = itertools.accumulate(sizes)
    return [(end - size, size) for end, size in zip(ends, sizes)]


def _for_rows(start, size, fn):
    if size <= 2 * _TILE:
        for r in range(start, start + size, _TILE):
            fn(pl.ds(r, _TILE))
        return

    @pl.loop(0, size // _TILE)
    def _(i):
        fn(pl.ds(pl.multiple_of(start + i * _TILE, _TILE), _TILE))


def _kernel(
    x_hbm, o_hbm,
    x_v, s1, r1, s2, r2, y_v, o_v,
    load_sem, r1_sem, r2_sem, g1_sem, g2_sem, g3_sem, send_sem, store_sem,
):
    q = x_hbm.shape[0] // 8
    halves = (0, 1)

    me = lax.axis_index("i")
    bit_x = me >> 1
    bit_y = (me ^ bit_x) & 1
    nbr_x, nbr_y = me ^ 3, me ^ 1
    partner1, partner2 = (nbr_x, nbr_y), (nbr_y, nbr_x)
    bit1, bit2 = (bit_x, bit_y), (bit_y, bit_x)

    def hbm_rows(h, flip1, flip2, start, size):
        quarter = 4 * h + 2 * (bit1[h] ^ flip1) + (bit2[h] ^ flip2)
        return pl.ds(pl.multiple_of(quarter * q + start, _TILE), size)

    def remote(src, dst, snd, rcv, to):
        return pltpu.make_async_remote_copy(
            src, dst, snd, rcv, device_id=(to,),
            device_id_type=pl.DeviceIdType.MESH,
        )

    in_flips = ((1, 1), (1, 0), (0, 1), (0, 0))
    rs1 = [(0, *s) for s in _spans(_RS1_FIRST)] + [(1, *s) for s in _spans(_RS1_SECOND)]
    loads = rs1 + [(2, 0, q), (3, 0, q)]

    def load(h, k):
        slot, start, size = loads[k]
        return pltpu.make_async_copy(
            x_hbm.at[hbm_rows(h, *in_flips[slot], start, size)],
            x_v.at[h, slot, pl.ds(start, size)],
            load_sem.at[h * len(loads) + k],
        )

    out_flips = ((0, 0), (0, 1), (1, 0), (1, 1))

    def store(h, slot, start, size):
        pltpu.make_async_copy(
            o_v.at[h, slot, pl.ds(start, size)],
            o_hbm.at[hbm_rows(h, *out_flips[slot], start, size)],
            store_sem,
        ).start()

    def widen_and_store(h, slot, start, size):
        def widen(rows):
            o_v[h, slot, rows] = y_v[h, slot, rows].astype(jnp.float32)

        _for_rows(start, size, widen)
        store(h, slot, start, size)

    def rs1_copy(h, k):
        slot, start, size = rs1[k]
        rows = pl.ds(start, size)
        return remote(s1.at[h, slot, rows], r1.at[h, slot, rows], send_sem.at[0],
                      r1_sem.at[h * len(rs1) + k], partner1[h])

    rs2 = _spans(_RS2)

    def rs2_copy(h, k):
        rows = pl.ds(*rs2[k])
        return remote(s2.at[h, rows], r2.at[h, rows], send_sem.at[1],
                      r2_sem.at[h * len(rs2) + k], partner2[h])

    def ag1_copy(h, start, size):
        rows = pl.ds(start, size)
        return remote(y_v.at[h, 0, rows], y_v.at[h, 1, rows], send_sem.at[2],
                      g1_sem.at[h], partner2[h])

    def ag2_own_copy(h):
        return remote(y_v.at[h, 0], y_v.at[h, 2], send_sem.at[3],
                      g2_sem.at[h], partner1[h])

    ag2 = _spans(_AG2_LAST)

    def ag2_fwd_copy(h, k):
        rows = pl.ds(*ag2[k])
        return remote(y_v.at[h, 1, rows], y_v.at[h, 3, rows], send_sem.at[4],
                      g3_sem.at[h * len(ag2) + k], partner1[h])

    def wait_sent(ref, sem):
        pltpu.make_async_copy(ref, ref, sem).wait()

    for h in halves:
        load(h, 0).start()
    barrier = pltpu.get_barrier_semaphore()
    for nbr in (nbr_x, nbr_y):
        pl.semaphore_signal(barrier, 1, device_id=(nbr,),
                            device_id_type=pl.DeviceIdType.MESH)
    for k in range(1, len(loads)):
        for h in halves:
            load(h, k).start()

    for k, (slot, start, size) in enumerate(rs1):
        for h in halves:
            load(h, k).wait()

            def narrow(rows):
                s1[h, slot, rows] = x_v[h, slot, rows].astype(jnp.bfloat16)

            _for_rows(start, size, narrow)
            if k == 0 and h == 0:
                pl.semaphore_wait(barrier, 2)
            rs1_copy(h, k).start()

    for h in halves:
        load(h, len(rs1)).wait()
        for k in range(len(_RS1_FIRST)):
            rs1_copy(h, k).wait_recv()

        def partial_sum(rows):
            total = x_v[h, 2, rows] + r1[h, 0, rows].astype(jnp.float32)
            s2[h, rows] = total.astype(jnp.bfloat16)

        _for_rows(0, q, partial_sum)
        for k in range(len(rs2)):
            rs2_copy(h, k).start()

    for h in halves:
        load(h, len(rs1) + 1).wait()
        for k in range(len(_RS1_FIRST), len(rs1)):
            rs1_copy(h, k).wait_recv()
    for k, (start, size) in enumerate(rs2):
        for h in halves:
            rs2_copy(h, k).wait_recv()

            def finish(rows):
                s = (x_v[h, 3, rows] + r1[h, 1, rows].astype(jnp.float32)
                     + r2[h, rows].astype(jnp.float32))
                r = jnp.maximum(s, 0.0)
                y = jnp.tanh(s) * s * s + r * r * r
                y_v[h, 0, rows] = y.astype(jnp.bfloat16)

            _for_rows(start, size, finish)
            ag1_copy(h, start, size).start()

    for h in halves:
        ag2_own_copy(h).start()
    for h in halves:
        widen_and_store(h, 0, 0, q)
    wait_sent(s1, send_sem.at[0])
    wait_sent(s2, send_sem.at[1])
    for h in halves:
        ag1_copy(h, 0, q).wait_recv()
        for k in range(len(ag2)):
            ag2_fwd_copy(h, k).start()
    for h in halves:
        widen_and_store(h, 1, 0, q)
    wait_sent(y_v.at[:, 0], send_sem.at[2])
    for h in halves:
        ag2_own_copy(h).wait_recv()
        widen_and_store(h, 2, 0, q)
    wait_sent(y_v.at[:, 0], send_sem.at[3])
    for k, (start, size) in enumerate(ag2):
        if k == len(ag2) - 1:
            wait_sent(y_v.at[:, 1], send_sem.at[4])
        for h in halves:
            ag2_fwd_copy(h, k).wait_recv()
            widen_and_store(h, 3, start, size)
    pltpu.make_async_copy(o_v, o_v, store_sem).wait()


def pallas_dist_f_of_ar_i_m4096_n1024_kernel(t: jax.Array):
    m, n = t.shape
    q = m // 8
    assert sum(_RS1_FIRST) == sum(_RS1_SECOND) == sum(_RS2) == sum(_AG2_LAST) == q
    n_rs1 = len(_RS1_FIRST) + len(_RS1_SECOND)
    dma = pltpu.SemaphoreType.DMA
    return pl.pallas_call(
        _kernel,
        out_shape=jax.ShapeDtypeStruct((m, n), jnp.float32),
        in_specs=[pl.BlockSpec(memory_space=pl.ANY)],
        out_specs=pl.BlockSpec(memory_space=pl.ANY),
        scratch_shapes=[
            pltpu.VMEM((2, 4, q, n), jnp.float32),
            pltpu.VMEM((2, 2, q, n), jnp.bfloat16),
            pltpu.VMEM((2, 2, q, n), jnp.bfloat16),
            pltpu.VMEM((2, q, n), jnp.bfloat16),
            pltpu.VMEM((2, q, n), jnp.bfloat16),
            pltpu.VMEM((2, 4, q, n), jnp.bfloat16),
            pltpu.VMEM((2, 4, q, n), jnp.float32),
            dma((2 * (n_rs1 + 2),)),
            dma((2 * n_rs1,)),
            dma((2 * len(_RS2),)),
            dma((2,)),
            dma((2,)),
            dma((2 * len(_AG2_LAST),)),
            dma((5,)),
            dma(()),
        ],
        compiler_params=pltpu.CompilerParams(
            collective_id=0, vmem_limit_bytes=96 * 1024 * 1024
        ),
    )(t)
```

```python
import itertools

import jax
import jax.numpy as jnp
from jax import lax
from jax.experimental import pallas as pl
from jax.experimental.pallas import tpu as pltpu

_TILE = 16

_RS1_FIRST = (16, 32, 80, 128, 256)
_RS1_SECOND = (512,)
_RS2 = (128, 128, 128, 128)


def _spans(sizes):
    ends = itertools.accumulate(sizes)
    return [(end - size, size) for end, size in zip(ends, sizes)]


def _for_tiles(start, size, fn):
    if size <= 2 * _TILE:
        for row in range(start, start + size, _TILE):
            fn(row)
        return

    @pl.loop(0, size // _TILE)
    def _(i):
        fn(pl.multiple_of(start + i * _TILE, _TILE))


def _kernel(
    x_hbm, out,
    x_v, s1, r1, s2, r2,
    load_sem, r1_sem, r2_sem, gather_sem, send_sem,
):
    q = x_hbm.shape[0] // 8
    halves = (0, 1)

    me = lax.axis_index("i")
    bit_x = me >> 1
    bit_y = (me ^ bit_x) & 1
    nbr_x, nbr_y = me ^ 3, me ^ 1
    partner1, partner2 = (nbr_x, nbr_y), (nbr_y, nbr_x)
    bit1, bit2 = (bit_x, bit_y), (bit_y, bit_x)

    def global_rows(h, flip1, flip2, start, size):
        quarter = 4 * h + 2 * (bit1[h] ^ flip1) + (bit2[h] ^ flip2)
        return pl.ds(pl.multiple_of(quarter * q + start, _TILE), size)

    def remote(src, dst, snd, rcv, to):
        return pltpu.make_async_remote_copy(
            src, dst, snd, rcv, device_id=(to,),
            device_id_type=pl.DeviceIdType.MESH,
        )

    flips = ((1, 1), (1, 0), (0, 1), (0, 0))
    rs1 = [(0, *s) for s in _spans(_RS1_FIRST)] + [(1, *s) for s in _spans(_RS1_SECOND)]
    rs2 = _spans(_RS2)
    loads = rs1 + [(2, 0, q), (3, 0, q)]

    def load(h, k):
        slot, start, size = loads[k]
        return pltpu.make_async_copy(
            x_hbm.at[global_rows(h, *flips[slot], start, size)],
            x_v.at[h, slot, pl.ds(start, size)],
            load_sem.at[h * len(loads) + k],
        )

    def rs1_copy(h, k):
        slot, start, size = rs1[k]
        rows = pl.ds(start, size)
        return remote(s1.at[h, slot, rows], r1.at[h, slot, rows], send_sem.at[0],
                      r1_sem.at[h * len(rs1) + k], partner1[h])

    def rs2_copy(h, k):
        rows = pl.ds(*rs2[k])
        return remote(s2.at[h, rows], r2.at[h, rows], send_sem.at[1],
                      r2_sem.at[h * len(rs2) + k], partner2[h])

    def gather_copy(h, stage, flip1, flip2, start=0, size=q):
        rows = out.at[global_rows(h, flip1, flip2, start, size)]
        return remote(rows, rows, send_sem.at[2 + 3 * h + stage],
                      gather_sem.at[3 * h + stage],
                      partner2[h] if stage == 0 else partner1[h])

    for h in halves:
        load(h, 0).start()
    barrier = pltpu.get_barrier_semaphore()
    for nbr in (nbr_x, nbr_y):
        pl.semaphore_signal(barrier, 1, device_id=(nbr,),
                            device_id_type=pl.DeviceIdType.MESH)
    for k in range(1, len(loads)):
        for h in halves:
            load(h, k).start()

    for k, (slot, start, size) in enumerate(rs1):
        for h in halves:
            load(h, k).wait()

            def narrow(row):
                rows = pl.ds(row, _TILE)
                s1[h, slot, rows] = x_v[h, slot, rows].astype(jnp.bfloat16)

            _for_tiles(start, size, narrow)
            if k == 0 and h == 0:
                pl.semaphore_wait(barrier, 2)
            rs1_copy(h, k).start()

    for h in halves:
        load(h, len(rs1)).wait()
        for k in range(len(_RS1_FIRST)):
            rs1_copy(h, k).wait_recv()

        def partial_sum(row):
            rows = pl.ds(row, _TILE)
            total = x_v[h, 2, rows] + r1[h, 0, rows].astype(jnp.float32)
            s2[h, rows] = total.astype(jnp.bfloat16)

        _for_tiles(0, q, partial_sum)
        for k in range(len(rs2)):
            rs2_copy(h, k).start()

    for h in halves:
        load(h, len(rs1) + 1).wait()
        for k in range(len(_RS1_FIRST), len(rs1)):
            rs1_copy(h, k).wait_recv()
    for k, (start, size) in enumerate(rs2):
        for h in halves:
            rs2_copy(h, k).wait_recv()

            def finish(row):
                rows = pl.ds(row, _TILE)
                s = (x_v[h, 3, rows] + r1[h, 1, rows].astype(jnp.float32)
                     + r2[h, rows].astype(jnp.float32))
                r = jnp.maximum(s, 0.0)
                y = jnp.tanh(s) * s * s + r * r * r
                out[global_rows(h, 0, 0, row, _TILE)] = y.astype(out.dtype)

            _for_tiles(start, size, finish)
            gather_copy(h, 0, 0, 0, start, size).start()

    for h in halves:
        gather_copy(h, 1, 0, 0).start()
    for h in halves:
        gather_copy(h, 0, 0, 1).wait_recv()
        gather_copy(h, 2, 0, 1).start()

    pltpu.make_async_copy(s1, s1, send_sem.at[0]).wait()
    pltpu.make_async_copy(s2, s2, send_sem.at[1]).wait()
    for h in halves:
        gather_copy(h, 0, 0, 0).wait_send()
        gather_copy(h, 1, 0, 0).wait_send()
        gather_copy(h, 1, 1, 0).wait_recv()
    for h in halves:
        gather_copy(h, 2, 0, 1).wait_send()
    for h in halves:
        gather_copy(h, 2, 1, 1).wait_recv()


def pallas_dist_f_of_ar_i_m4096_n1024_kernel(t: jax.Array):
    m, n = t.shape
    q = m // 8
    assert sum(_RS1_FIRST) == sum(_RS1_SECOND) == sum(_RS2) == q
    n_rs1 = len(_RS1_FIRST) + len(_RS1_SECOND)
    dma = pltpu.SemaphoreType.DMA
    return pl.pallas_call(
        _kernel,
        out_shape=jax.ShapeDtypeStruct((m, n), jnp.bfloat16),
        in_specs=[pl.BlockSpec(memory_space=pltpu.HBM)],
        out_specs=pl.BlockSpec(memory_space=pltpu.VMEM),
        scratch_shapes=[
            pltpu.VMEM((2, 4, q, n), jnp.float32),
            pltpu.VMEM((2, 2, q, n), jnp.bfloat16),
            pltpu.VMEM((2, 2, q, n), jnp.bfloat16),
            pltpu.VMEM((2, q, n), jnp.bfloat16),
            pltpu.VMEM((2, q, n), jnp.bfloat16),
            dma((2 * (n_rs1 + 2),)),
            dma((2 * n_rs1,)),
            dma((2 * len(_RS2),)),
            dma((6,)),
            dma((8,)),
        ],
        compiler_params=pltpu.CompilerParams(
            collective_id=0, vmem_limit_bytes=48 * 1024 * 1024
        ),
    )(t)
```

```python
import itertools

import jax
import jax.numpy as jnp
from jax import lax
from jax.experimental import pallas as pl
from jax.experimental.pallas import tpu as pltpu

_TILE = 16

_RS1_CHUNKS = (16, 48, 128, 320)
_RS2_CHUNKS = (256, 256)


def _spans(sizes):
    ends = itertools.accumulate(sizes)
    return [(end - size, size) for end, size in zip(ends, sizes)]


def _for_tiles(start, size, fn):
    @pl.loop(0, size // _TILE)
    def _(i):
        fn(pl.multiple_of(start + i * _TILE, _TILE))


def _wait_filled(ref, sem):
    pltpu.make_async_copy(ref, ref, sem).wait()


def _kernel(
    x_hbm, out,
    x_v, snd, rcv,
    load_sem, rs_send_sem, rs1_sem, rs2_sem, ag_send_sem, ag_sem,
):
    q = x_hbm.shape[0] // 8
    halves = (0, 1)

    me = lax.axis_index("i")
    bit_x = me >> 1
    bit_y = (me ^ bit_x) & 1
    nbr_x, nbr_y = me ^ 3, me ^ 1
    partner1, partner2 = (nbr_x, nbr_y), (nbr_y, nbr_x)
    bit1, bit2 = (bit_x, bit_y), (bit_y, bit_x)

    def quarter(h, flip1, flip2, start=0, size=q):
        index = 4 * h + 2 * (bit1[h] ^ flip1) + (bit2[h] ^ flip2)
        return pl.ds(pl.multiple_of(index * q + start, _TILE), size)

    def quarter_pair(h, flip1):
        index = 4 * h + 2 * (bit1[h] ^ flip1)
        return pl.ds(pl.multiple_of(index * q, _TILE), 2 * q)

    def send(src, dst, send_sem, recv_sem, to):
        pltpu.make_async_remote_copy(
            src, dst, send_sem, recv_sem, device_id=(to,),
            device_id_type=pl.DeviceIdType.MESH,
        ).start()

    def wait_sent(ref, send_sem):
        pltpu.make_async_remote_copy(
            ref, ref, send_sem, send_sem, device_id=(nbr_x,),
            device_id_type=pl.DeviceIdType.MESH,
        ).wait_send()

    flips = ((1, 1), (1, 0), (0, 1), (0, 0))
    rs1 = [(0, *span) for span in _spans(_RS1_CHUNKS)] + [(1, 0, q)]
    rs2 = _spans(_RS2_CHUNKS)

    def load(slot, start, size, sem):
        for h in halves:
            pltpu.make_async_copy(
                x_hbm.at[quarter(h, *flips[slot], start, size)],
                x_v.at[slot, h, pl.ds(start, size)], sem,
            ).start()

    barrier = pltpu.get_barrier_semaphore()
    for nbr in (nbr_x, nbr_y):
        pl.semaphore_signal(barrier, 1, device_id=(nbr,),
                            device_id_type=pl.DeviceIdType.MESH)
    for k, chunk in enumerate(rs1):
        load(*chunk, load_sem.at[k])

    for k, (slot, start, size) in enumerate(rs1):
        rows = pl.ds(start, size)
        _wait_filled(x_v.at[slot, :, rows], load_sem.at[k])

        def narrow(row):
            tile = pl.ds(row, _TILE)
            snd[slot, :, tile] = x_v[slot, :, tile].astype(snd.dtype)

        _for_tiles(start, size, narrow)
        if k == 0:
            pl.semaphore_wait(barrier, 2)
        for h in halves:
            send(snd.at[slot, h, rows], rcv.at[slot, h, rows],
                 rs_send_sem, rs1_sem.at[slot], partner1[h])

    for slot in (2, 3):
        load(slot, 0, q, load_sem.at[len(rs1)])
    _wait_filled(x_v.at[2:], load_sem.at[len(rs1)])
    _wait_filled(rcv.at[0], rs1_sem.at[0])

    def partial_sum(row):
        tile = pl.ds(row, _TILE)
        total = x_v[2, :, tile] + rcv[0, :, tile].astype(jnp.float32)
        snd[2, :, tile] = total.astype(snd.dtype)

    _for_tiles(0, q, partial_sum)
    for k, (start, size) in enumerate(rs2):
        rows = pl.ds(start, size)
        for h in halves:
            send(snd.at[2, h, rows], rcv.at[2, h, rows],
                 rs_send_sem, rs2_sem.at[k], partner2[h])

    def finish(row):
        tile = pl.ds(row, _TILE)
        for h in halves:
            s = (x_v[3, h, tile] + rcv[1, h, tile].astype(jnp.float32)
                 + rcv[2, h, tile].astype(jnp.float32))
            r = jnp.maximum(s, 0.0)
            y = jnp.tanh(s) * s * s + r * r * r
            out[quarter(h, 0, 0, row, _TILE)] = y.astype(out.dtype)

    def gather(h, stage, rows, to):
        send(out.at[rows], out.at[rows], ag_send_sem.at[2 * stage + h],
             ag_sem.at[2 * stage + h], to)

    _wait_filled(rcv.at[1], rs1_sem.at[1])
    for k, (start, size) in enumerate(rs2):
        _wait_filled(rcv.at[2, :, pl.ds(start, size)], rs2_sem.at[k])
        _for_tiles(start, size, finish)
        for h in halves:
            gather(h, 0, quarter(h, 0, 0, start, size), partner2[h])

    for h in halves:
        gather(h, 1, quarter(h, 0, 0), partner1[h])
    for h in halves:
        _wait_filled(out.at[quarter(h, 0, 1)], ag_sem.at[h])
        gather(h, 1, quarter(h, 0, 1), partner1[h])

    wait_sent(snd, rs_send_sem)
    for h in halves:
        wait_sent(out.at[quarter(h, 0, 0)], ag_send_sem.at[h])
    for h in halves:
        wait_sent(out.at[quarter_pair(h, 0)], ag_send_sem.at[2 + h])
    for h in halves:
        _wait_filled(out.at[quarter_pair(h, 1)], ag_sem.at[2 + h])


def pallas_dist_f_of_ar_i_m4096_n1024_kernel(t: jax.Array):
    m, n = t.shape
    q = m // 8
    assert m == 8 * q and sum(_RS1_CHUNKS) == sum(_RS2_CHUNKS) == q
    dma = pltpu.SemaphoreType.DMA
    return pl.pallas_call(
        _kernel,
        out_shape=jax.ShapeDtypeStruct((m, n), jnp.bfloat16),
        in_specs=[pl.BlockSpec(memory_space=pltpu.HBM)],
        out_specs=pl.BlockSpec(memory_space=pltpu.VMEM),
        scratch_shapes=[
            pltpu.VMEM((4, 2, q, n), jnp.float32),
            pltpu.VMEM((3, 2, q, n), jnp.bfloat16),
            pltpu.VMEM((3, 2, q, n), jnp.bfloat16),
            dma((len(_RS1_CHUNKS) + 2,)),
            dma(()),
            dma((2,)),
            dma((len(_RS2_CHUNKS),)),
            dma((4,)),
            dma((4,)),
        ],
        compiler_params=pltpu.CompilerParams(
            collective_id=0, vmem_limit_bytes=48 * 1024 * 1024
        ),
    )(t)
```
